```python
import numpy as np
kernel_name = 'dist_attn_cross_mha_kvrep_htp_ss_b1_sq512_skv2048_d1024_hq8_dh128'

def setup_inputs():
    x = np.random.randn(1, 2048, 1024).astype(np.float32)
    Wq = np.random.randn(1024, 4096).astype(np.float32) * 0.02
    K_ext = np.random.randn(1, 2048, 32, 128).astype(np.float32)
    V_ext = np.random.randn(1, 2048, 32, 128).astype(np.float32)
    Wo = np.random.randn(4096, 1024).astype(np.float32) * 0.02
    return {'x': x, 'Wq': Wq, 'K_ext': K_ext, 'V_ext': V_ext, 'Wo': Wo}

def reference(x, Wq, K_ext, V_ext, Wo):
    B, Sq, Hq, Hkv, Dh = (1, 2048, 32, 32, 128)
    Q = (x @ Wq).reshape(B, Sq, Hq, Dh)
    K, V = (K_ext, V_ext)
    Skv = K.shape[1]
    out = np.zeros((B, Sq, Hq, Dh), dtype=np.float32)
    m = np.full((B, Hq, Sq, 1), -np.inf, dtype=np.float32)
    l = np.zeros((B, Hq, Sq, 1), dtype=np.float32)
    for j0 in range(0, Skv, 1024):
        Kj = K[:, j0:j0 + 1024].copy()
        Vj = V[:, j0:j0 + 1024].copy()
        sj = np.einsum('bihd,bjhd->bhij', Q, Kj).astype(np.float32) * 0.08838834764831843
        mj = sj.max(axis=-1, keepdims=True)
        m_new = np.maximum(m, mj)
        alpha = np.exp(m - m_new)
        pj = np.exp(sj - m_new)
        l = l * alpha + pj.sum(axis=-1, keepdims=True)
        out = out * alpha.transpose(0, 2, 1, 3) + np.einsum('bhij,bjhd->bihd', pj, Vj)
        m = m_new
    out = (out / l.transpose(0, 2, 1, 3)).reshape(B, Sq, Hq * Dh)
    return out @ Wo
```

```python
import jax
import jax.numpy as jnp
from jax import lax
from jax.experimental import pallas as pl
from jax.experimental.pallas import tpu as pltpu

N_DEV = 4
H = 8
DH = 128
SKV = 2048
SQ = 512
DM = 1024
BQ = 256
HB = 128
N_SUB = 6

QSCALE = 0.08838834764831843 * 1.4426950408889634

_NT = (((1,), (1,)), ((), ()))
BF16 = jnp.bfloat16
F32 = jnp.float32


def _attend(q, k, v):
    s = lax.dot_general(q, k, _NT, preferred_element_type=F32)
    m = jnp.max(s, axis=-1, keepdims=True)
    p = jnp.exp2(s - m)
    l = jnp.sum(p, axis=-1, keepdims=True)
    o = jnp.dot(p.astype(BF16), v, preferred_element_type=F32)
    r = pl.reciprocal(l, approx=True)
    r = r * (2.0 - l * r)
    return (o * r).astype(BF16)


def _kernel(x_hbm, wq_hbm, k_hbm, v_hbm, wo_hbm, out_hbm,
            xf, xown, xg, wqf, wqb, wof, wob, kf, vf, kb, vb,
            oown, pbuf, rbuf, outf,
            x_sem, wq_sem, k_sem, v_sem, wo_sem, out_sem,
            ag_send, ag_recv, rs_send, rs_recv):
    my = lax.axis_index("i")
    left = lax.rem(my + N_DEV - 1, N_DEV)
    right = lax.rem(my + 1, N_DEV)
    h0 = my * H

    def x_copy(u):
        return pltpu.make_async_copy(
            x_hbm.at[0, pl.ds(u * BQ, BQ), :], xf.at[u], x_sem.at[u])

    def wq_copy(h):
        return pltpu.make_async_copy(
            wq_hbm.at[:, pl.ds(h * DH, DH)], wqf.at[h], wq_sem.at[h])

    def k_copy(h):
        return pltpu.make_async_copy(
            k_hbm.at[0, :, h0 + h, :], kf.at[h], k_sem.at[h])

    def v_copy(h):
        return pltpu.make_async_copy(
            v_hbm.at[0, :, h0 + h, :], vf.at[h], v_sem.at[h])

    wo_copy = pltpu.make_async_copy(wo_hbm, wof, wo_sem.at[0])

    def out_copy(u):
        return pltpu.make_async_copy(
            outf.at[u], out_hbm.at[0, pl.ds(u * BQ, BQ), :], out_sem.at[u])

    x_copy(0).start()
    x_copy(1).start()
    for h in range(H):
        wq_copy(h).start()
        k_copy(h).start()
        v_copy(h).start()
    wo_copy.start()

    barrier = pltpu.get_barrier_semaphore()
    for nbr in (left, right):
        pl.semaphore_signal(barrier, inc=1, device_id=(nbr,),
                            device_id_type=pl.DeviceIdType.MESH)

    def ag_copy(src, s, part, dev):
        idx = 2 * s + part
        return pltpu.make_async_remote_copy(
            src_ref=src, dst_ref=xg.at[s, pl.ds(part * HB, HB), :],
            send_sem=ag_send.at[idx], recv_sem=ag_recv.at[idx],
            device_id=(dev,), device_id_type=pl.DeviceIdType.MESH)

    def ag_own(u, stage):
        da, db = (left, right) if stage == 0 else (right, left)
        s = 2 * stage + u
        return (ag_copy(xown.at[u, pl.ds(0, HB), :], s, 0, da),
                ag_copy(xown.at[u, pl.ds(HB, HB), :], s, 1, db))

    def ag_fwd(u):
        return (ag_copy(xg.at[u, pl.ds(0, HB), :], 2 + u, 0, left),
                ag_copy(xg.at[u, pl.ds(HB, HB), :], 2 + u, 1, right))

    def rs_copy(s, part, dev):
        idx = 2 * s + part
        return pltpu.make_async_remote_copy(
            src_ref=pbuf.at[s, pl.ds(part * HB, HB), :],
            dst_ref=rbuf.at[s, pl.ds(part * HB, HB), :],
            send_sem=rs_send.at[idx], recv_sem=rs_recv.at[idx],
            device_id=(dev,), device_id_type=pl.DeviceIdType.MESH)

    def ag_wait_recv(s):
        for part in range(2):
            ag_copy(xg.at[s, pl.ds(part * HB, HB), :], s, part, my).wait_recv()

    def rs_wait_recv(s):
        for part in range(2):
            rs_copy(s, part, my).wait_recv()

    rbuf[N_SUB] = jnp.zeros((BQ, DM), BF16)

    for u in range(2):
        x_copy(u).wait()
        xown[u] = xf[u].astype(BF16)

    pl.semaphore_wait(barrier, 2)
    for stage in (0, 2):
        for u in range(2):
            for c in ag_own(u, stage):
                c.start()

    for h in range(H):
        wq_copy(h).wait()
        k_copy(h).wait()
        v_copy(h).wait()
        w = wqf[h].astype(BF16)
        wqb[:, h * DH:(h + 1) * DH] = w
        k = kf[h].astype(BF16)
        kb[h] = k
        v = vf[h].astype(BF16)
        vb[h] = v
        for u in range(2):
            q = jnp.dot(xown[u], w, preferred_element_type=F32) * QSCALE
            oown[u, :, h * DH:(h + 1) * DH] = _attend(q.astype(BF16), k, v)

    wo_copy.wait()
    wob[...] = wof[...].astype(BF16)

    def sub_block(s, carry):
        ag_wait_recv(s)

        @pl.when(s < 2)
        def _():
            for c in ag_fwd(s):
                c.start()

        @pl.when(s >= 4)
        def _():
            rs_wait_recv(s - 2)

        up = jnp.where(s >= 4, s - 2, N_SUB)
        q = jnp.dot(xg[s], wqb[...], preferred_element_type=F32) * QSCALE
        q = q.astype(BF16)
        o = jnp.concatenate(
            [_attend(q[:, h * DH:(h + 1) * DH], kb[h], vb[h]) for h in range(H)],
            axis=-1)
        y = jnp.dot(o, wob[...], preferred_element_type=F32)
        pbuf[s] = (y + rbuf[up].astype(F32)).astype(BF16)
        first = s < 2
        rs_copy(s, 0, jnp.where(first, right, left)).start()
        rs_copy(s, 1, jnp.where(first, left, right)).start()
        return carry

    lax.fori_loop(0, N_SUB, sub_block, 0)

    for u in range(2):
        rs_wait_recv(u)
    rs_wait_recv(4)
    y0 = jnp.dot(oown[0], wob[...], preferred_element_type=F32)
    outf[0] = y0 + rbuf[0].astype(F32) + rbuf[4].astype(F32)
    out_copy(0).start()
    y1 = jnp.dot(oown[1], wob[...], preferred_element_type=F32)
    outf[1] = y1 + rbuf[1].astype(F32)
    rs_wait_recv(5)
    outf[1] = outf[1] + rbuf[5].astype(F32)
    out_copy(1).start()

    for stage in (0, 2):
        for u in range(2):
            for c in ag_own(u, stage):
                c.wait_send()
    for u in range(2):
        for c in ag_fwd(u):
            c.wait_send()
    for s in range(N_SUB):
        for part in range(2):
            rs_copy(s, part, my).wait_send()
    out_copy(0).wait()
    out_copy(1).wait()


def pallas_dist_attn_cross_mha_kvrep_htp_ss_b1_sq512_skv2048_d1024_hq8_dh128_kernel(
    x: jax.Array,
    Wq: jax.Array,
    K_ext: jax.Array,
    V_ext: jax.Array,
    Wo: jax.Array,
):
    any_spec = pl.BlockSpec(memory_space=pl.ANY)
    return pl.pallas_call(
        _kernel,
        out_shape=jax.ShapeDtypeStruct((1, SQ, DM), F32),
        in_specs=[any_spec] * 5,
        out_specs=any_spec,
        scratch_shapes=[
            pltpu.VMEM((2, BQ, DM), F32),
            pltpu.VMEM((2, BQ, DM), BF16),
            pltpu.VMEM((N_SUB, BQ, DM), BF16),
            pltpu.VMEM((H, DM, DH), F32),
            pltpu.VMEM((DM, DM), BF16),
            pltpu.VMEM((DM, DM), F32),
            pltpu.VMEM((DM, DM), BF16),
            pltpu.VMEM((H, SKV, DH), F32),
            pltpu.VMEM((H, SKV, DH), F32),
            pltpu.VMEM((H, SKV, DH), BF16),
            pltpu.VMEM((H, SKV, DH), BF16),
            pltpu.VMEM((2, BQ, DM), BF16),
            pltpu.VMEM((N_SUB, BQ, DM), BF16),
            pltpu.VMEM((N_SUB + 1, BQ, DM), BF16),
            pltpu.VMEM((2, BQ, DM), F32),
            pltpu.SemaphoreType.DMA((2,)),
            pltpu.SemaphoreType.DMA((H,)),
            pltpu.SemaphoreType.DMA((H,)),
            pltpu.SemaphoreType.DMA((H,)),
            pltpu.SemaphoreType.DMA((1,)),
            pltpu.SemaphoreType.DMA((2,)),
            pltpu.SemaphoreType.DMA((2 * N_SUB,)),
            pltpu.SemaphoreType.DMA((2 * N_SUB,)),
            pltpu.SemaphoreType.DMA((2 * N_SUB,)),
            pltpu.SemaphoreType.DMA((2 * N_SUB,)),
        ],
        compiler_params=pltpu.CompilerParams(
            collective_id=0,
            vmem_limit_bytes=100 * 1024 * 1024,
        ),
    )(x, Wq, K_ext, V_ext, Wo)
```

```python
import jax
import jax.numpy as jnp
from jax import lax
from jax.experimental import pallas as pl
from jax.experimental.pallas import tpu as pltpu

N_DEV = 4
H = 8
DH = 128
SKV = 2048
SQ = 512
DM = 1024
BQ = 256
HB = 128
N_SUB = 6
NWC = 4
WC = DM // NWC
HPC = WC // DH
QSCALE = 0.08838834764831843 * 1.4426950408889634
_NT = (((1,), (1,)), ((), ()))
BF16 = jnp.bfloat16
F32 = jnp.float32


def _dot(a, b):
    return jnp.dot(a, b, preferred_element_type=F32)


def _scores(q, k):
    return lax.dot_general(q, k, _NT, preferred_element_type=F32)


def _pv(s, v):
    m = jnp.max(s, axis=-1, keepdims=True)
    p = jnp.exp2(s - m)
    lp = p[:, 0:DH]
    for j in range(1, SKV // DH):
        lp = lp + p[:, j * DH:(j + 1) * DH]
    return _dot(p.astype(BF16), v), lp


def _norm(o, lp):
    l = jnp.sum(lp, axis=-1, keepdims=True)
    return (o * pl.reciprocal(l, approx=True)).astype(BF16)


def _attend(q, k, v):
    s = _scores(q, k)
    m = jnp.max(s, axis=-1, keepdims=True)
    p = jnp.exp2(s - m)
    l = jnp.sum(p, axis=-1, keepdims=True)
    o = _dot(p.astype(BF16), v)
    return (o * pl.reciprocal(l, approx=True)).astype(BF16)


def _kernel(x_hbm, wq_hbm, k_hbm, v_hbm, wo_hbm, out_ref,
            xf, xown, xg, wqf, wqb, wof, wob, kf, vf, kb, vb,
            q1, o1, ou, lp, pbuf, rbuf,
            ld_sem, ag_send, ag_recv, rs_send, rs_recv):
    my = lax.axis_index("i")
    left = lax.rem(my + N_DEV - 1, N_DEV)
    right = lax.rem(my + 1, N_DEV)
    h0 = my * H

    barrier = pltpu.get_barrier_semaphore()
    for nbr in (left, right):
        pl.semaphore_signal(barrier, inc=1, device_id=(nbr,),
                            device_id_type=pl.DeviceIdType.MESH)

    def x_copy(u):
        return pltpu.make_async_copy(
            x_hbm.at[0, pl.ds(u * BQ, BQ), :], xf.at[pl.ds(u * BQ, BQ), :], ld_sem.at[u])

    def wq_copy(c):
        return pltpu.make_async_copy(
            wq_hbm.at[:, pl.ds(c * WC, WC)], wqf.at[c], ld_sem.at[2 + c])

    def k_copy(h):
        return pltpu.make_async_copy(
            k_hbm.at[0, :, h0 + h, :], kf.at[h], ld_sem.at[2 + NWC + 2 * h])

    def v_copy(h):
        return pltpu.make_async_copy(
            v_hbm.at[0, :, h0 + h, :], vf.at[h], ld_sem.at[3 + NWC + 2 * h])

    wo_copy = pltpu.make_async_copy(wo_hbm, wof, ld_sem.at[2 + NWC + 2 * H])

    x_copy(0).start(priority=1)
    x_copy(1).start(priority=1)
    for c in range(NWC):
        wq_copy(c).start(priority=1)
    for h in range(H):
        k_copy(h).start(priority=1)
        v_copy(h).start(priority=1)
    wo_copy.start(priority=1)

    def ag_copy(src, s, part, dev):
        idx = 2 * s + part
        return pltpu.make_async_remote_copy(
            src_ref=src, dst_ref=xg.at[s, pl.ds(part * HB, HB), :],
            send_sem=ag_send.at[idx], recv_sem=ag_recv.at[idx],
            device_id=(dev,), device_id_type=pl.DeviceIdType.MESH)

    def ag_own(u, stage):
        da, db = (left, right) if stage == 0 else (right, left)
        s = 2 * stage + u
        return (ag_copy(xown.at[pl.ds(u * BQ, HB), :], s, 0, da),
                ag_copy(xown.at[pl.ds(u * BQ + HB, HB), :], s, 1, db))

    def ag_fwd(u):
        return (ag_copy(xg.at[u, pl.ds(0, HB), :], 2 + u, 0, left),
                ag_copy(xg.at[u, pl.ds(HB, HB), :], 2 + u, 1, right))

    def rs_copy(s, part, dev):
        idx = 2 * s + part
        return pltpu.make_async_remote_copy(
            src_ref=pbuf.at[s, pl.ds(part * HB, HB), :],
            dst_ref=rbuf.at[s, pl.ds(part * HB, HB), :],
            send_sem=rs_send.at[idx], recv_sem=rs_recv.at[idx],
            device_id=(dev,), device_id_type=pl.DeviceIdType.MESH)

    def ag_wait_recv(s):
        for part in range(2):
            ag_copy(xg.at[s, pl.ds(part * HB, HB), :], s, part, my).wait_recv()

    def rs_wait_recv(s):
        for part in range(2):
            rs_copy(s, part, my).wait_recv()

    rbuf[N_SUB] = jnp.zeros((BQ, DM), BF16)
    ou[...] = jnp.zeros(ou.shape, F32)
    lp[...] = jnp.ones(lp.shape, F32)

    x_copy(0).wait()
    xown[0:BQ, :] = xf[0:BQ, :].astype(BF16)
    pl.semaphore_wait(barrier, 2)
    for c in ag_own(0, 0):
        c.start()
    x_copy(1).wait()
    xown[BQ:SQ, :] = xf[BQ:SQ, :].astype(BF16)

    for c in range(NWC):
        wq_copy(c).wait()
        w = wqf[c].astype(BF16)
        wqb[:, c * WC:(c + 1) * WC] = w
        q = (_dot(xown[...], w) * QSCALE).astype(BF16)
        for j in range(HPC):
            q1[c * HPC + j, 0:SQ, :] = q[:, j * DH:(j + 1) * DH]

    ag_wait_recv(0)
    for c in ag_own(1, 0):
        c.start()
    for c in ag_fwd(0):
        c.start()
    q = (_dot(xg[0], wqb[...]) * QSCALE).astype(BF16)
    for h in range(H):
        q1[h, SQ:SQ + BQ, :] = q[:, h * DH:(h + 1) * DH]

    def load_kv(h):
        k_copy(h).wait()
        v_copy(h).wait()
        k = kf[h].astype(BF16)
        kb[h] = k
        v = vf[h].astype(BF16)
        vb[h] = v
        return k, v

    def norm_prev(slot):
        for g in range(3):
            o1[slot, g * BQ:(g + 1) * BQ, :] = _norm(ou[g], lp[g])

    def head(h, carry):
        k, v = load_kv(h)
        norm_prev(h)
        for g in range(3):
            o, l = _pv(_scores(q1[h, g * BQ:(g + 1) * BQ, :], k), v)
            ou[g] = o
            lp[g] = l
        return carry

    lax.fori_loop(0, H - 1, head, 0)

    hl = H - 1

    def o_rows(g, k, v):
        last = _norm(*_pv(_scores(q1[hl, g * BQ:(g + 1) * BQ, :], k), v))
        return jnp.concatenate(
            [o1[h + 1, g * BQ:(g + 1) * BQ, :] for h in range(hl)] + [last], axis=-1)

    for u in range(2):
        for c in ag_own(u, 2):
            c.start()
    wo_copy.wait()
    k, v = load_kv(hl)
    norm_prev(hl)
    w = wof[...].astype(BF16)
    wob[...] = w
    pbuf[0] = _dot(o_rows(2, k, v), w).astype(BF16)
    rs_copy(0, 0, right).start()
    rs_copy(0, 1, left).start()

    def sub_block(s, carry):
        ag_wait_recv(s)

        @pl.when(s == 1)
        def _():
            for c in ag_fwd(1):
                c.start()

        @pl.when(s >= 4)
        def _():
            rs_wait_recv(s - 2)

        up = jnp.where(s >= 4, s - 2, N_SUB)
        q = (_dot(xg[s], wqb[...]) * QSCALE).astype(BF16)
        o = jnp.concatenate(
            [_attend(q[:, h * DH:(h + 1) * DH], kb[h], vb[h]) for h in range(H)], axis=-1)
        pbuf[s] = (_dot(o, wob[...]) + rbuf[up].astype(F32)).astype(BF16)
        first = s < 2
        rs_copy(s, 0, jnp.where(first, right, left)).start()
        rs_copy(s, 1, jnp.where(first, left, right)).start()
        return carry

    lax.fori_loop(1, N_SUB, sub_block, 0)

    for s in (0, 1, 4):
        rs_wait_recv(s)
    og = [o_rows(g, kb[hl], vb[hl]) for g in range(2)]
    for g in range(2):
        y = _dot(og[g], wob[...]) + rbuf[g].astype(F32)
        if g == 0:
            y = y + rbuf[4].astype(F32)
        out_ref[0, g * BQ:(g + 1) * BQ, :] = y
    rs_wait_recv(5)
    out_ref[0, BQ:SQ, :] = out_ref[0, BQ:SQ, :] + rbuf[5].astype(F32)

    for stage in (0, 2):
        for u in range(2):
            for c in ag_own(u, stage):
                c.wait_send()
    for u in range(2):
        for c in ag_fwd(u):
            c.wait_send()
    for s in range(N_SUB):
        for part in range(2):
            rs_copy(s, part, my).wait_send()


def pallas_dist_attn_cross_mha_kvrep_htp_ss_b1_sq512_skv2048_d1024_hq8_dh128_kernel(x, Wq, K_ext, V_ext, Wo):
    any_spec = pl.BlockSpec(memory_space=pl.ANY)
    return pl.pallas_call(
        _kernel,
        out_shape=jax.ShapeDtypeStruct((1, SQ, DM), F32),
        in_specs=[any_spec] * 5,
        out_specs=pl.BlockSpec(memory_space=pltpu.VMEM),
        scratch_shapes=[
            pltpu.VMEM((SQ, DM), F32),
            pltpu.VMEM((SQ, DM), BF16),
            pltpu.VMEM((N_SUB, BQ, DM), BF16),
            pltpu.VMEM((NWC, DM, WC), F32),
            pltpu.VMEM((DM, DM), BF16),
            pltpu.VMEM((DM, DM), F32),
            pltpu.VMEM((DM, DM), BF16),
            pltpu.VMEM((H, SKV, DH), F32),
            pltpu.VMEM((H, SKV, DH), F32),
            pltpu.VMEM((H, SKV, DH), BF16),
            pltpu.VMEM((H, SKV, DH), BF16),
            pltpu.VMEM((H, 3 * BQ, DH), BF16),
            pltpu.VMEM((H, 3 * BQ, DH), BF16),
            pltpu.VMEM((3, BQ, DH), F32),
            pltpu.VMEM((3, BQ, DH), F32),
            pltpu.VMEM((N_SUB, BQ, DM), BF16),
            pltpu.VMEM((N_SUB + 1, BQ, DM), BF16),
            pltpu.SemaphoreType.DMA((3 + NWC + 2 * H,)),
            pltpu.SemaphoreType.DMA((2 * N_SUB,)),
            pltpu.SemaphoreType.DMA((2 * N_SUB,)),
            pltpu.SemaphoreType.DMA((2 * N_SUB,)),
            pltpu.SemaphoreType.DMA((2 * N_SUB,)),
        ],
        compiler_params=pltpu.CompilerParams(
            collective_id=0,
            vmem_limit_bytes=100 * 1024 * 1024,
            disable_bounds_checks=True,
            disable_semaphore_checks=True,
        ),
    )(x, Wq, K_ext, V_ext, Wo)
```

```python
import jax
import jax.numpy as jnp
from jax import lax
from jax.experimental import pallas as pl
from jax.experimental.pallas import tpu as pltpu

N_DEV = 4
H = 8
DH = 128
SKV = 2048
SQ = 512
DM = 1024
BQ = 256
HB = 128
N_SUB = 6
NP = 4
QB = BQ // NP
NWC = 8
WC = DM // NWC
NL = 6

QSCALE = 0.08838834764831843 * 1.4426950408889634

_NT = (((1,), (1,)), ((), ()))
BF16 = jnp.bfloat16
F32 = jnp.float32


def _dot(a, b):
    return jnp.dot(a, b, preferred_element_type=F32)


def _probs(q, k):
    s = lax.dot_general(q, k, _NT, preferred_element_type=F32)
    return jnp.exp2(s - jnp.max(s, axis=-1, keepdims=True))


def _recip_sum(p):
    return pl.reciprocal(jnp.sum(p, axis=-1, keepdims=True), approx=True)


def _attend_raw(q, k, v):
    p = _probs(q, k)
    lp = p[:, 0:DH]
    for j in range(1, SKV // DH):
        lp = lp + p[:, j * DH:(j + 1) * DH]
    return _dot(p.astype(BF16), v), lp


def _norm(o, lp):
    return (o * _recip_sum(lp)).astype(BF16)


def _kernel(x_hbm, wq_hbm, k_hbm, v_hbm, wo_hbm, out_ref,
            x0f, x1f, xown, xg, wqf, wqb, wof, wob, kf, vf, kb, vb,
            qacc, o1, ou, lp, pbuf, rbuf,
            ld_sem, ag_send, ag_recv, rs_send, rs_recv):
    my = lax.axis_index("i")
    left = lax.rem(my + N_DEV - 1, N_DEV)
    right = lax.rem(my + 1, N_DEV)
    h0 = my * H

    barrier = pltpu.get_barrier_semaphore()
    for nbr in (left, right):
        pl.semaphore_signal(barrier, inc=1, device_id=(nbr,),
                            device_id_type=pl.DeviceIdType.MESH)

    def piece_row(i):
        return (i % 2) * HB + (i // 2) * QB

    def x0_copy(i):
        rows = pl.ds(piece_row(i), QB)
        return pltpu.make_async_copy(
            x_hbm.at[0, rows, :], x0f.at[rows, :], ld_sem.at[i])

    def x1_copy(c):
        return pltpu.make_async_copy(
            x_hbm.at[0, pl.ds(BQ, BQ), pl.ds(c * WC, WC)], x1f.at[c],
            ld_sem.at[NP + 2 * c])

    def wq_copy(c):
        rows = pl.ds(c * WC, WC)
        return pltpu.make_async_copy(
            wq_hbm.at[rows, :], wqf.at[rows, :], ld_sem.at[NP + 2 * c + 1])

    def k_copy(h):
        return pltpu.make_async_copy(
            k_hbm.at[0, :, h0 + h, :], kf.at[h], ld_sem.at[NP + 2 * NWC + 2 * h])

    def v_copy(h):
        return pltpu.make_async_copy(
            v_hbm.at[0, :, h0 + h, :], vf.at[h],
            ld_sem.at[NP + 2 * NWC + 2 * h + 1])

    wo_copy = pltpu.make_async_copy(wo_hbm, wof, ld_sem.at[NP + 2 * NWC + 2 * H])

    for i in range(NP):
        x0_copy(i).start(priority=1)
    for c in range(NWC):
        x1_copy(c).start(priority=1)
        wq_copy(c).start(priority=1)

    def remote(src, dst, send_sem, recv_sem, dev):
        return pltpu.make_async_remote_copy(
            src_ref=src, dst_ref=dst, send_sem=send_sem, recv_sem=recv_sem,
            device_id=(dev,), device_id_type=pl.DeviceIdType.MESH)

    def first_copy(i, dev):
        rows = pl.ds(piece_row(i), QB)
        idx = i if i < 2 else 2 * N_SUB + i - 2
        return remote(xown.at[rows, :], xg.at[0, rows, :],
                      ag_send.at[idx], ag_recv.at[idx], dev)

    def ag_copy(src, s, part, dev):
        idx = 2 * s + part
        return remote(src, xg.at[s, pl.ds(part * HB, HB), :],
                      ag_send.at[idx], ag_recv.at[idx], dev)

    def ag_own(stage, u):
        d0, d1 = (left, right) if stage == 0 else (right, left)
        s = 2 * stage + u
        return (ag_copy(xown.at[pl.ds(u * BQ, HB), :], s, 0, d0),
                ag_copy(xown.at[pl.ds(u * BQ + HB, HB), :], s, 1, d1))

    def ag_fwd(u):
        return (ag_copy(xg.at[u, pl.ds(0, HB), :], 2 + u, 0, left),
                ag_copy(xg.at[u, pl.ds(HB, HB), :], 2 + u, 1, right))

    def rs_copy(s, part, dev):
        idx = 2 * s + part
        rows = pl.ds(part * HB, HB)
        return remote(pbuf.at[s, rows, :], rbuf.at[s, rows, :],
                      rs_send.at[idx], rs_recv.at[idx], dev)

    def ag_wait_recv(s):
        for part in range(2):
            ag_copy(xg.at[s, pl.ds(part * HB, HB), :], s, part, my).wait_recv()

    def rs_wait_recv(s):
        for part in range(2):
            rs_copy(s, part, my).wait_recv()

    rbuf[N_SUB] = jnp.zeros((BQ, DM), BF16)
    qacc[0:SQ, :] = jnp.zeros((SQ, DM), F32)
    ou[...] = jnp.zeros(ou.shape, F32)
    lp[...] = jnp.ones(lp.shape, F32)

    for i in range(NP):
        x0_copy(i).wait()
        r = piece_row(i)
        xown[r:r + QB, :] = x0f[r:r + QB, :].astype(BF16)
        if i == 0:
            pl.semaphore_wait(barrier, 2)
        first_copy(i, left if i % 2 == 0 else right).start()

    for h in range(H):
        k_copy(h).start(priority=1)
        v_copy(h).start(priority=1)
    wo_copy.start(priority=1)

    def q_chunk(c, carry):
        x1_copy(c).wait()
        wq_copy(c).wait()
        cs = pl.ds(pl.multiple_of(c * WC, WC), WC)
        x1 = x1f[c].astype(BF16)
        xown[BQ:SQ, cs] = x1
        w = (wqf[cs, :] * QSCALE).astype(BF16)
        wqb[cs, :] = w
        xc = jnp.concatenate([xown[0:BQ, cs], x1], axis=0)
        qacc[0:SQ, :] = qacc[0:SQ, :] + _dot(xc, w)
        return carry

    lax.fori_loop(0, NWC, q_chunk, 0)

    for i in range(NP):
        first_copy(i, my).wait_recv()
    for c in ag_own(0, 1) + ag_fwd(0):
        c.start()
    qacc[SQ:SQ + BQ, :] = _dot(xg[0], wqb[...])

    def q_rows(g, h):
        col = h * DH if isinstance(h, int) else pl.multiple_of(h * DH, DH)
        return qacc[g * BQ:(g + 1) * BQ, pl.ds(col, DH)].astype(BF16)

    def wait_kv(h):
        k_copy(h).wait()
        v_copy(h).wait()

    def cast_kv(h):
        k = kf[h].astype(BF16)
        kb[h] = k
        v = vf[h].astype(BF16)
        vb[h] = v
        return k, v

    def stash(g, h, k, v):
        o, l = _attend_raw(q_rows(g, h), k, v)
        ou[g] = o
        lp[g] = l

    def norm_prev(slot):
        for g in range(3):
            o1[slot, g * BQ:(g + 1) * BQ, :] = _norm(ou[g], lp[g])

    def head(h, carry):
        wait_kv(h)
        k, v = cast_kv(h)
        norm_prev(h)
        for g in range(3):
            stash(g, h, k, v)
        return carry

    lax.fori_loop(0, NL, head, 0)

    def attend(g, h, k, v):
        return _norm(*_attend_raw(q_rows(g, h), k, v))

    def o_cat(g, extra):
        return jnp.concatenate(
            [o1[h + 1, g * BQ:(g + 1) * BQ, :] for h in range(NL)] + extra, axis=-1)

    for u in range(2):
        for c in ag_own(2, u):
            c.start()
    wo_copy.wait()
    for h in range(NL, H):
        wait_kv(h)
    kv = {h: cast_kv(h) for h in range(NL, H)}
    norm_prev(NL)
    tail = [attend(2, h, *kv[h]) for h in range(NL, H)]
    stash(0, NL, *kv[NL])
    w = wof[...].astype(BF16)
    wob[...] = w
    pbuf[0] = _dot(o_cat(2, tail), w).astype(BF16)
    rs_copy(0, 0, right).start()
    rs_copy(0, 1, left).start()

    def sub_block(s, carry):
        ag_wait_recv(s)

        @pl.when(s == 1)
        def _():
            for c in ag_fwd(1):
                c.start()

        @pl.when(s >= 4)
        def _():
            rs_wait_recv(s - 2)

        q = _dot(xg[s], wqb[...]).astype(BF16)
        heads = []
        for h in range(H):
            p = _probs(q[:, h * DH:(h + 1) * DH], kb[h])
            r = _recip_sum(p)
            heads.append((_dot(p.astype(BF16), vb[h]).astype(BF16), r))
        y = rbuf[jnp.where(s >= 4, s - 2, N_SUB)].astype(F32)
        for h, (o, r) in enumerate(heads):
            y = y + _dot(o, wob[h * DH:(h + 1) * DH, :]) * r
        pbuf[s] = y.astype(BF16)
        first = s < 2
        rs_copy(s, 0, jnp.where(first, right, left)).start()
        rs_copy(s, 1, jnp.where(first, left, right)).start()
        return carry

    lax.fori_loop(1, N_SUB, sub_block, 0)

    for s in (0, 1, 4):
        rs_wait_recv(s)
    hl = H - 1
    tail0 = [_norm(ou[0], lp[0])]
    tail0 += [attend(0, h, kb[h], vb[h]) for h in range(NL + 1, H)]
    tail1 = [attend(1, h, kb[h], vb[h]) for h in range(NL, hl)]
    stash(1, hl, kb[hl], vb[hl])
    out_ref[0, 0:BQ, :] = (_dot(o_cat(0, tail0), wob[...])
                           + rbuf[0].astype(F32) + rbuf[4].astype(F32))
    out_ref[0, BQ:SQ, :] = (_dot(o_cat(1, tail1), wob[0:hl * DH, :])
                            + rbuf[1].astype(F32))
    rs_wait_recv(5)
    y = _dot(ou[1].astype(BF16), wob[hl * DH:, :]) * _recip_sum(lp[1])
    out_ref[0, BQ:SQ, :] = out_ref[0, BQ:SQ, :] + rbuf[5].astype(F32) + y

    for i in range(NP):
        first_copy(i, my).wait_send()
    for c in (ag_own(0, 1) + ag_own(2, 0) + ag_own(2, 1)
              + ag_fwd(0) + ag_fwd(1)):
        c.wait_send()
    for s in range(N_SUB):
        for part in range(2):
            rs_copy(s, part, my).wait_send()


def pallas_dist_attn_cross_mha_kvrep_htp_ss_b1_sq512_skv2048_d1024_hq8_dh128_kernel(
    x: jax.Array,
    Wq: jax.Array,
    K_ext: jax.Array,
    V_ext: jax.Array,
    Wo: jax.Array,
):
    any_spec = pl.BlockSpec(memory_space=pl.ANY)
    n_ag = 2 * N_SUB + NP - 2
    return pl.pallas_call(
        _kernel,
        out_shape=jax.ShapeDtypeStruct((1, SQ, DM), F32),
        in_specs=[any_spec] * 5,
        out_specs=pl.BlockSpec(memory_space=pltpu.VMEM),
        scratch_shapes=[
            pltpu.VMEM((BQ, DM), F32),
            pltpu.VMEM((NWC, BQ, WC), F32),
            pltpu.VMEM((SQ, DM), BF16),
            pltpu.VMEM((N_SUB, BQ, DM), BF16),
            pltpu.VMEM((DM, DM), F32),
            pltpu.VMEM((DM, DM), BF16),
            pltpu.VMEM((DM, DM), F32),
            pltpu.VMEM((DM, DM), BF16),
            pltpu.VMEM((H, SKV, DH), F32),
            pltpu.VMEM((H, SKV, DH), F32),
            pltpu.VMEM((H, SKV, DH), BF16),
            pltpu.VMEM((H, SKV, DH), BF16),
            pltpu.VMEM((3 * BQ, DM), F32),
            pltpu.VMEM((NL + 1, 3 * BQ, DH), BF16),
            pltpu.VMEM((3, BQ, DH), F32),
            pltpu.VMEM((3, BQ, DH), F32),
            pltpu.VMEM((N_SUB, BQ, DM), BF16),
            pltpu.VMEM((N_SUB + 1, BQ, DM), BF16),
            pltpu.SemaphoreType.DMA((NP + 2 * NWC + 2 * H + 1,)),
            pltpu.SemaphoreType.DMA((n_ag,)),
            pltpu.SemaphoreType.DMA((n_ag,)),
            pltpu.SemaphoreType.DMA((2 * N_SUB,)),
            pltpu.SemaphoreType.DMA((2 * N_SUB,)),
        ],
        compiler_params=pltpu.CompilerParams(
            collective_id=0,
            vmem_limit_bytes=100 * 1024 * 1024,
            disable_bounds_checks=True,
            disable_semaphore_checks=True,
        ),
    )(x, Wq, K_ext, V_ext, Wo)
```

```python
import jax
import jax.numpy as jnp
from jax import lax
from jax.experimental import pallas as pl
from jax.experimental.pallas import tpu as pltpu

N_DEV = 4
H = 8
DH = 128
SKV = 2048
SQ = 512
DM = 1024
BQ = 256
HB = 128
N_SUB = 6
NP = 4
QB = BQ // NP
NWC = 8
WC = DM // NWC
NL = 6
R1 = 3 * BQ
CUT = 304

QSCALE = 0.08838834764831843 * 1.4426950408889634

_NT = (((1,), (1,)), ((), ()))
BF16 = jnp.bfloat16
F32 = jnp.float32


def _dot(a, b):
    return jnp.dot(a, b, preferred_element_type=F32)


def _scores(q, k):
    return lax.dot_general(q, k, _NT, preferred_element_type=F32)


def _exp_shifted(s):
    return jnp.exp2(s - jnp.max(s, axis=-1, keepdims=True))


def _recip_sum(p):
    return pl.reciprocal(jnp.sum(p, axis=-1, keepdims=True), approx=True)


def _attend_raw(q, k, v):
    p = _exp_shifted(_scores(q, k))
    lp = p[:, 0:DH]
    for j in range(1, SKV // DH):
        lp = lp + p[:, j * DH:(j + 1) * DH]
    return _dot(p.astype(BF16), v), lp


def _norm(o, lp):
    return (o * _recip_sum(lp)).astype(BF16)


def _kernel(x_hbm, wq_hbm, k_hbm, v_hbm, wo_hbm, out_ref,
            x0f, x1f, xown, xg, wqf, wqb, wof, wob, kf, vf, kb, vb,
            qacc, o1, ou, lp, pbuf, rbuf,
            ld_sem, ag_send, ag_recv, rs_send, rs_recv):
    my = lax.axis_index("i")
    left = lax.rem(my + N_DEV - 1, N_DEV)
    right = lax.rem(my + 1, N_DEV)
    h0 = my * H

    def piece_row(i):
        return (i % 2) * HB + (i // 2) * QB

    def x0_copy(i):
        rows = pl.ds(piece_row(i), QB)
        return pltpu.make_async_copy(
            x_hbm.at[0, rows, :], x0f.at[rows, :], ld_sem.at[i])

    def x1_copy(c):
        return pltpu.make_async_copy(
            x_hbm.at[0, pl.ds(BQ, BQ), pl.ds(c * WC, WC)], x1f.at[c],
            ld_sem.at[NP + 2 * c])

    def wq_copy(c):
        rows = pl.ds(c * WC, WC)
        return pltpu.make_async_copy(
            wq_hbm.at[rows, :], wqf.at[rows, :], ld_sem.at[NP + 2 * c + 1])

    def k_copy(h):
        return pltpu.make_async_copy(
            k_hbm.at[0, :, h0 + h, :], kf.at[h], ld_sem.at[NP + 2 * NWC + 2 * h])

    def v_copy(h):
        return pltpu.make_async_copy(
            v_hbm.at[0, :, h0 + h, :], vf.at[h],
            ld_sem.at[NP + 2 * NWC + 2 * h + 1])

    def wo_copy():
        return pltpu.make_async_copy(
            wo_hbm, wof, ld_sem.at[NP + 2 * NWC + 2 * H])

    def remote(src, dst, send_sem, recv_sem, dev):
        return pltpu.make_async_remote_copy(
            src_ref=src, dst_ref=dst, send_sem=send_sem, recv_sem=recv_sem,
            device_id=(dev,), device_id_type=pl.DeviceIdType.MESH)

    def first_copy(i, dev):
        rows = pl.ds(piece_row(i), QB)
        idx = i if i < 2 else 2 * N_SUB + i - 2
        return remote(xown.at[rows, :], xg.at[0, rows, :],
                      ag_send.at[idx], ag_recv.at[idx], dev)

    def ag_copy(src, s, part, dev):
        idx = 2 * s + part
        return remote(src, xg.at[s, pl.ds(part * HB, HB), :],
                      ag_send.at[idx], ag_recv.at[idx], dev)

    def ag_own(stage, u):
        d0, d1 = (left, right) if stage == 0 else (right, left)
        s = 2 * stage + u
        return (ag_copy(xown.at[pl.ds(u * BQ, HB), :], s, 0, d0),
                ag_copy(xown.at[pl.ds(u * BQ + HB, HB), :], s, 1, d1))

    def ag_fwd(u):
        return (ag_copy(xg.at[u, pl.ds(0, HB), :], 2 + u, 0, left),
                ag_copy(xg.at[u, pl.ds(HB, HB), :], 2 + u, 1, right))

    def rs_copy(s, part, dev):
        idx = 2 * s + part
        rows = pl.ds(part * HB, HB)
        return remote(pbuf.at[s, rows, :], rbuf.at[s, rows, :],
                      rs_send.at[idx], rs_recv.at[idx], dev)

    def ag_wait_recv(s):
        for part in range(2):
            ag_copy(xg.at[s, pl.ds(part * HB, HB), :], s, part, my).wait_recv()

    def rs_wait_recv(s):
        for part in range(2):
            rs_copy(s, part, my).wait_recv()

    def q_rows(a, b, h):
        col = h * DH if isinstance(h, int) else pl.multiple_of(h * DH, DH)
        return qacc[a:b, pl.ds(col, DH)].astype(BF16)

    def attend(g, h, k, v):
        return _norm(*_attend_raw(q_rows(g * BQ, (g + 1) * BQ, h), k, v))

    def stash(a, b, h, k, v):
        o, l = _attend_raw(q_rows(a, b, h), k, v)
        ou[a:b, :] = o
        lp[a:b, :] = l

    def o_cat(g, extra):
        return jnp.concatenate(
            [o1[h + 1, g * BQ:(g + 1) * BQ, :] for h in range(NL)] + extra, axis=-1)

    def streaming_phase():
        barrier = pltpu.get_barrier_semaphore()
        for nbr in (left, right):
            pl.semaphore_signal(barrier, inc=1, device_id=(nbr,),
                                device_id_type=pl.DeviceIdType.MESH)
        for i in range(NP):
            x0_copy(i).start(priority=1)
        for c in range(NWC):
            x1_copy(c).start(priority=1)
            wq_copy(c).start(priority=1)

        rbuf[N_SUB] = jnp.zeros((BQ, DM), BF16)
        qacc[0:SQ, :] = jnp.zeros((SQ, DM), F32)
        ou[...] = jnp.zeros(ou.shape, F32)
        lp[...] = jnp.ones(lp.shape, F32)

        for i in range(NP):
            x0_copy(i).wait()
            r = piece_row(i)
            xown[r:r + QB, :] = x0f[r:r + QB, :].astype(BF16)
            if i == 0:
                pl.semaphore_wait(barrier, 2)
            first_copy(i, left if i % 2 == 0 else right).start()

        for h in range(H):
            k_copy(h).start(priority=1)
            v_copy(h).start(priority=1)
        wo_copy().start(priority=1)

        def q_chunk(c, carry):
            x1_copy(c).wait()
            wq_copy(c).wait()
            cs = pl.ds(pl.multiple_of(c * WC, WC), WC)
            x1 = x1f[c].astype(BF16)
            xown[BQ:SQ, cs] = x1
            w = (wqf[cs, :] * QSCALE).astype(BF16)
            for h in range(H):
                wqb[h, cs, :] = w[:, h * DH:(h + 1) * DH]
            xc = jnp.concatenate([xown[0:BQ, cs], x1], axis=0)
            qacc[0:SQ, :] = qacc[0:SQ, :] + _dot(xc, w)
            return carry

        lax.fori_loop(0, NWC, q_chunk, 0)

        for i in range(NP):
            first_copy(i, my).wait_recv()
        for c in ag_own(0, 1) + ag_fwd(0):
            c.start()
        qacc[SQ:R1, :] = _dot(
            xg[0], jnp.concatenate([wqb[h] for h in range(H)], axis=-1))

        def wait_kv(h):
            k_copy(h).wait()
            v_copy(h).wait()

        def cast_kv(h):
            k = kf[h].astype(BF16)
            kb[h] = k
            v = vf[h].astype(BF16)
            vb[h] = v
            return k, v

        def head(h, carry):
            wait_kv(h)
            k, v = cast_kv(h)
            o1[h] = _norm(ou[...], lp[...])
            stash(0, CUT, h, k, v)
            stash(CUT, R1, h, k, v)
            return carry

        lax.fori_loop(0, NL, head, 0)

        for c in ag_own(2, 0) + ag_own(2, 1):
            c.start()
        wo_copy().wait()
        for h in range(NL, H):
            wait_kv(h)
        kv = {h: cast_kv(h) for h in range(NL, H)}
        o1[NL] = _norm(ou[...], lp[...])
        tail = [attend(2, h, *kv[h]) for h in range(NL, H)]
        stash(0, BQ, NL, *kv[NL])
        w = wof[...].astype(BF16)
        wob[...] = w
        pbuf[0] = _dot(o_cat(2, tail), w).astype(BF16)
        rs_copy(0, 0, right).start()
        rs_copy(0, 1, left).start()

    def sub_block(s, carry):
        ag_wait_recv(s)

        @pl.when(s == 1)
        def _():
            for c in ag_fwd(1):
                c.start()

        @pl.when(s >= 4)
        def _():
            rs_wait_recv(s - 2)

        x = xg[s]
        q = [_dot(x, wqb[h]).astype(BF16) for h in range(2)]
        heads = []
        for h in range(H):
            sc = _scores(q[h], kb[h])
            if 1 <= h < H - 1:
                q.append(_dot(x, wqb[h + 1]).astype(BF16))
            p = _exp_shifted(sc)
            r = _recip_sum(p)
            heads.append((_dot(p.astype(BF16), vb[h]).astype(BF16), r))
        y = rbuf[jnp.where(s >= 4, s - 2, N_SUB)].astype(F32)
        for h, (o, r) in enumerate(heads):
            y = y + _dot(o, wob[h * DH:(h + 1) * DH, :]) * r
        pbuf[s] = y.astype(BF16)
        first = s < 2
        rs_copy(s, 0, jnp.where(first, right, left)).start()
        rs_copy(s, 1, jnp.where(first, left, right)).start()
        return carry

    def steady_phase():
        lax.fori_loop(1, N_SUB, sub_block, 0)

        for s in (0, 1, 4):
            rs_wait_recv(s)
        hl = H - 1
        tail0 = [_norm(ou[0:BQ, :], lp[0:BQ, :])]
        tail0 += [attend(0, h, kb[h], vb[h]) for h in range(NL + 1, H)]
        tail1 = [attend(1, h, kb[h], vb[h]) for h in range(NL, hl)]
        stash(BQ, SQ, hl, kb[hl], vb[hl])
        out_ref[0, 0:BQ, :] = (_dot(o_cat(0, tail0), wob[...])
                               + rbuf[0].astype(F32) + rbuf[4].astype(F32))
        out_ref[0, BQ:SQ, :] = (_dot(o_cat(1, tail1), wob[0:hl * DH, :])
                                + rbuf[1].astype(F32))
        for i in range(NP):
            first_copy(i, my).wait_send()
        for c in (ag_own(0, 1) + ag_own(2, 0) + ag_own(2, 1)
                  + ag_fwd(0) + ag_fwd(1)):
            c.wait_send()
        for s in range(N_SUB):
            for part in range(2):
                rs_copy(s, part, my).wait_send()
        rs_wait_recv(5)
        y = _dot(ou[BQ:SQ, :].astype(BF16), wob[hl * DH:, :])
        y = y * _recip_sum(lp[BQ:SQ, :])
        out_ref[0, BQ:SQ, :] = out_ref[0, BQ:SQ, :] + rbuf[5].astype(F32) + y

    def phase(i, carry):
        pl.when(i == 0)(streaming_phase)
        pl.when(i == 1)(steady_phase)
        return carry

    lax.fori_loop(0, 2, phase, 0)


def pallas_dist_attn_cross_mha_kvrep_htp_ss_b1_sq512_skv2048_d1024_hq8_dh128_kernel(
    x: jax.Array,
    Wq: jax.Array,
    K_ext: jax.Array,
    V_ext: jax.Array,
    Wo: jax.Array,
):
    any_spec = pl.BlockSpec(memory_space=pl.ANY)
    n_ag = 2 * N_SUB + NP - 2
    return pl.pallas_call(
        _kernel,
        out_shape=jax.ShapeDtypeStruct((1, SQ, DM), F32),
        in_specs=[any_spec] * 5,
        out_specs=pl.BlockSpec(memory_space=pltpu.VMEM),
        scratch_shapes=[
            pltpu.VMEM((BQ, DM), F32),
            pltpu.VMEM((NWC, BQ, WC), F32),
            pltpu.VMEM((SQ, DM), BF16),
            pltpu.VMEM((N_SUB, BQ, DM), BF16),
            pltpu.VMEM((DM, DM), F32),
            pltpu.VMEM((H, DM, DH), BF16),
            pltpu.VMEM((DM, DM), F32),
            pltpu.VMEM((DM, DM), BF16),
            pltpu.VMEM((H, SKV, DH), F32),
            pltpu.VMEM((H, SKV, DH), F32),
            pltpu.VMEM((H, SKV, DH), BF16),
            pltpu.VMEM((H, SKV, DH), BF16),
            pltpu.VMEM((R1, DM), F32),
            pltpu.VMEM((NL + 1, R1, DH), BF16),
            pltpu.VMEM((R1, DH), F32),
            pltpu.VMEM((R1, DH), F32),
            pltpu.VMEM((N_SUB, BQ, DM), BF16),
            pltpu.VMEM((N_SUB + 1, BQ, DM), BF16),
            pltpu.SemaphoreType.DMA((NP + 2 * NWC + 2 * H + 1,)),
            pltpu.SemaphoreType.DMA((n_ag,)),
            pltpu.SemaphoreType.DMA((n_ag,)),
            pltpu.SemaphoreType.DMA((2 * N_SUB,)),
            pltpu.SemaphoreType.DMA((2 * N_SUB,)),
        ],
        compiler_params=pltpu.CompilerParams(
            collective_id=0,
            vmem_limit_bytes=100 * 1024 * 1024,
            disable_bounds_checks=True,
            disable_semaphore_checks=True,
        ),
    )(x, Wq, K_ext, V_ext, Wo)
```

```python
import jax
import jax.numpy as jnp
from jax import lax
from jax.experimental import pallas as pl
from jax.experimental.pallas import tpu as pltpu

N_DEV = 4
H = 8
DH = 128
SKV = 2048
SQ = 512
DM = 1024
BQ = 256
HB = 128
N_SUB = 6
NP = 4
QB = BQ // NP
NWC = 8
WC = DM // NWC
NL = H - 2
R1 = 3 * BQ
CUT = 304

QSCALE = 0.08838834764831843 * 1.4426950408889634

_NT = (((1,), (1,)), ((), ()))
BF16 = jnp.bfloat16
F32 = jnp.float32


def _dot(a, b):
    return jnp.dot(a, b, preferred_element_type=F32)


def _scores(q, k):
    return lax.dot_general(q, k, _NT, preferred_element_type=F32)


def _exp_shifted(s):
    return jnp.exp2(s - jnp.max(s, axis=-1, keepdims=True))


def _recip_sum(p):
    l = jnp.sum(p, axis=-1, keepdims=True)
    r = pl.reciprocal(l, approx=True)
    return r * (2.0 - l * r)


def _pv_raw(s, v):
    p = _exp_shifted(s)
    lp = p[:, 0:DH]
    for j in range(1, SKV // DH):
        lp = lp + p[:, j * DH:(j + 1) * DH]
    return _dot(p.astype(BF16), v), lp


def _norm(o, lp):
    return (o * _recip_sum(lp)).astype(BF16)


def _kernel(x_hbm, wq_hbm, k_hbm, v_hbm, wo_hbm, out_ref,
            x0f, x1f, xown, xg, wqf, wqb, wof, wob, kf, vf, kb, vb,
            qacc, o1, ou, lp, pbuf, rbuf,
            ld_sem, ag_send, ag_recv, rs_send, rs_recv):
    my = lax.axis_index("i")
    left = lax.rem(my + N_DEV - 1, N_DEV)
    right = lax.rem(my + 1, N_DEV)
    h0 = my * H

    def piece_row(i):
        return (i % 2) * HB + (i // 2) * QB

    def x0_copy(i):
        rows = pl.ds(piece_row(i), QB)
        return pltpu.make_async_copy(
            x_hbm.at[0, rows, :], x0f.at[rows, :], ld_sem.at[i])

    def x1_copy(c):
        return pltpu.make_async_copy(
            x_hbm.at[0, pl.ds(BQ, BQ), pl.ds(c * WC, WC)], x1f.at[c],
            ld_sem.at[NP + 2 * c])

    def wq_copy(c):
        rows = pl.ds(c * WC, WC)
        return pltpu.make_async_copy(
            wq_hbm.at[rows, :], wqf.at[rows, :], ld_sem.at[NP + 2 * c + 1])

    def k_copy(h):
        return pltpu.make_async_copy(
            k_hbm.at[0, :, h0 + h, :], kf.at[h], ld_sem.at[NP + 2 * NWC + 2 * h])

    def v_copy(h):
        return pltpu.make_async_copy(
            v_hbm.at[0, :, h0 + h, :], vf.at[h],
            ld_sem.at[NP + 2 * NWC + 2 * h + 1])

    def wo_copy():
        return pltpu.make_async_copy(
            wo_hbm, wof, ld_sem.at[NP + 2 * NWC + 2 * H])

    def remote(src, dst, send_sem, recv_sem, dev):
        return pltpu.make_async_remote_copy(
            src_ref=src, dst_ref=dst, send_sem=send_sem, recv_sem=recv_sem,
            device_id=(dev,), device_id_type=pl.DeviceIdType.MESH)

    def first_copy(i, dev):
        rows = pl.ds(piece_row(i), QB)
        idx = i if i < 2 else 2 * N_SUB + i - 2
        return remote(xown.at[rows, :], xg.at[0, rows, :],
                      ag_send.at[idx], ag_recv.at[idx], dev)

    def ag_copy(src, s, part, dev):
        idx = 2 * s + part
        return remote(src, xg.at[s, pl.ds(part * HB, HB), :],
                      ag_send.at[idx], ag_recv.at[idx], dev)

    def ag_own(stage, u):
        d0, d1 = (left, right) if stage == 0 else (right, left)
        s = 2 * stage + u
        return (ag_copy(xown.at[pl.ds(u * BQ, HB), :], s, 0, d0),
                ag_copy(xown.at[pl.ds(u * BQ + HB, HB), :], s, 1, d1))

    def ag_fwd(u):
        return (ag_copy(xg.at[u, pl.ds(0, HB), :], 2 + u, 0, left),
                ag_copy(xg.at[u, pl.ds(HB, HB), :], 2 + u, 1, right))

    def rs_copy(s, part, dev):
        idx = 2 * s + part
        rows = pl.ds(part * HB, HB)
        return remote(pbuf.at[s, rows, :], rbuf.at[s, rows, :],
                      rs_send.at[idx], rs_recv.at[idx], dev)

    def ag_wait_recv(s):
        for part in range(2):
            ag_copy(xg.at[s, pl.ds(part * HB, HB), :], s, part, my).wait_recv()

    def rs_wait_recv(s):
        for part in range(2):
            rs_copy(s, part, my).wait_recv()

    def q_rows(a, b, h):
        col = h * DH if isinstance(h, int) else pl.multiple_of(h * DH, DH)
        return qacc[a:b, pl.ds(col, DH)].astype(BF16)

    def attend(g, h, k, v):
        return _norm(*_pv_raw(_scores(q_rows(g * BQ, (g + 1) * BQ, h), k), v))

    def stash_pv(a, b, s, v):
        o, l = _pv_raw(s, v)
        ou[a:b, :] = o
        lp[a:b, :] = l

    def stash(a, b, h, k, v):
        stash_pv(a, b, _scores(q_rows(a, b, h), k), v)

    def o_head(g, h):
        return o1[h + 1, g * BQ:(g + 1) * BQ, :]

    def o_cat(g, first, extra):
        return jnp.concatenate(
            [o_head(g, h) for h in range(first, NL)] + extra, axis=-1)

    def streaming_phase():
        barrier = pltpu.get_barrier_semaphore()
        for nbr in (left, right):
            pl.semaphore_signal(barrier, inc=1, device_id=(nbr,),
                                device_id_type=pl.DeviceIdType.MESH)
        for i in range(NP):
            x0_copy(i).start(priority=1)
        for c in range(NWC):
            x1_copy(c).start(priority=1)
            wq_copy(c).start(priority=1)

        rbuf[N_SUB] = jnp.zeros((BQ, DM), BF16)
        qacc[0:SQ, :] = jnp.zeros((SQ, DM), F32)
        ou[...] = jnp.zeros(ou.shape, F32)
        lp[...] = jnp.ones(lp.shape, F32)

        for i in range(NP):
            x0_copy(i).wait()
            r = piece_row(i)
            xown[r:r + QB, :] = x0f[r:r + QB, :].astype(BF16)
            if i == 0:
                pl.semaphore_wait(barrier, 2)
            first_copy(i, left if i % 2 == 0 else right).start()

        for h in range(H):
            k_copy(h).start(priority=1)
            v_copy(h).start(priority=1)
        wo_copy().start(priority=1)

        def q_chunk(c, carry):
            x1_copy(c).wait()
            wq_copy(c).wait()
            cs = pl.ds(pl.multiple_of(c * WC, WC), WC)
            x1 = x1f[c].astype(BF16)
            xown[BQ:SQ, cs] = x1
            w = (wqf[cs, :] * QSCALE).astype(BF16)
            for h in range(H):
                wqb[h, cs, :] = w[:, h * DH:(h + 1) * DH]
            xc = jnp.concatenate([xown[0:BQ, cs], x1], axis=0)
            qacc[0:SQ, :] = qacc[0:SQ, :] + _dot(xc, w)
            return carry

        lax.fori_loop(0, NWC, q_chunk, 0)

        for i in range(NP):
            first_copy(i, my).wait_recv()
        for c in ag_own(0, 1) + ag_fwd(0):
            c.start()
        qacc[SQ:R1, :] = _dot(
            xg[0], jnp.concatenate([wqb[h] for h in range(H)], axis=-1))

        def wait_kv(h):
            k_copy(h).wait()
            v_copy(h).wait()

        def cast_kv(h):
            k = kf[h].astype(BF16)
            kb[h] = k
            v = vf[h].astype(BF16)
            vb[h] = v
            return k, v

        def head(h, carry):
            wait_kv(h)
            k, v = cast_kv(h)
            o1[h] = _norm(ou[...], lp[...])
            stash(0, CUT, h, k, v)
            stash(CUT, R1, h, k, v)
            return carry

        lax.fori_loop(0, NL, head, 0)

        for c in ag_own(2, 0) + ag_own(2, 1):
            c.start()
        wo_copy().wait()
        for h in range(NL, H):
            wait_kv(h)
        kv = {h: cast_kv(h) for h in range(NL, H)}
        o1[NL] = _norm(ou[...], lp[...])
        tail = [attend(2, h, *kv[h]) for h in range(NL, H)]
        stash(0, BQ, NL, *kv[NL])
        w = wof[...].astype(BF16)
        wob[...] = w
        pbuf[0] = _dot(o_cat(2, 0, tail), w).astype(BF16)
        rs_copy(0, 0, right).start()
        rs_copy(0, 1, left).start()

    def sub_block(s, carry):
        ag_wait_recv(s)

        @pl.when(s == 1)
        def _():
            for c in ag_fwd(1):
                c.start()

        @pl.when(s >= 4)
        def _():
            rs_wait_recv(s - 2)

        x = xg[s]
        q = [_dot(x, wqb[h]).astype(BF16) for h in range(2)]
        heads = []
        for h in range(H):
            sc = _scores(q[h], kb[h])
            if 1 <= h < H - 1:
                q.append(_dot(x, wqb[h + 1]).astype(BF16))
            p = _exp_shifted(sc)
            r = _recip_sum(p)
            heads.append((_dot(p.astype(BF16), vb[h]).astype(BF16), r))
        y = rbuf[jnp.where(s >= 4, s - 2, N_SUB)].astype(F32)
        for h, (o, r) in enumerate(heads):
            y = y + _dot(o, wob[h * DH:(h + 1) * DH, :]) * r
        pbuf[s] = y.astype(BF16)
        first = s < 2
        rs_copy(s, 0, jnp.where(first, right, left)).start()
        rs_copy(s, 1, jnp.where(first, left, right)).start()
        return carry

    def steady_phase():
        lax.fori_loop(1, N_SUB, sub_block, 0)

        for s in (0, 1, 4):
            rs_wait_recv(s)
        hl = H - 1
        y1 = rbuf[1].astype(F32) + _dot(o_head(1, 0), wob[0:DH, :])
        tail0 = [_norm(ou[0:BQ, :], lp[0:BQ, :]), attend(0, hl, kb[hl], vb[hl])]
        tail1 = [attend(1, NL, kb[NL], vb[NL])]
        sc = _scores(q_rows(BQ, SQ, hl), kb[hl])
        y1 = y1 + _dot(o_head(1, 1), wob[DH:2 * DH, :])
        stash_pv(BQ, SQ, sc, vb[hl])
        out_ref[0, 0:BQ, :] = (_dot(o_cat(0, 0, tail0), wob[...])
                               + rbuf[0].astype(F32) + rbuf[4].astype(F32))
        out_ref[0, BQ:SQ, :] = y1 + _dot(o_cat(1, 2, tail1), wob[2 * DH:hl * DH, :])
        for i in range(NP):
            first_copy(i, my).wait_send()
        for c in (ag_own(0, 1) + ag_own(2, 0) + ag_own(2, 1)
                  + ag_fwd(0) + ag_fwd(1)):
            c.wait_send()
        for s in range(N_SUB):
            for part in range(2):
                rs_copy(s, part, my).wait_send()
        rs_wait_recv(5)
        y = _dot(ou[BQ:SQ, :].astype(BF16), wob[hl * DH:, :])
        y = y * _recip_sum(lp[BQ:SQ, :])
        out_ref[0, BQ:SQ, :] = out_ref[0, BQ:SQ, :] + rbuf[5].astype(F32) + y

    def phase(i, carry):
        pl.when(i == 0)(streaming_phase)
        pl.when(i == 1)(steady_phase)
        return carry

    lax.fori_loop(0, 2, phase, 0)


def pallas_dist_attn_cross_mha_kvrep_htp_ss_b1_sq512_skv2048_d1024_hq8_dh128_kernel(
    x: jax.Array,
    Wq: jax.Array,
    K_ext: jax.Array,
    V_ext: jax.Array,
    Wo: jax.Array,
):
    any_spec = pl.BlockSpec(memory_space=pl.ANY)
    n_ag = 2 * N_SUB + NP - 2
    return pl.pallas_call(
        _kernel,
        out_shape=jax.ShapeDtypeStruct((1, SQ, DM), F32),
        in_specs=[any_spec] * 5,
        out_specs=pl.BlockSpec(memory_space=pltpu.VMEM),
        scratch_shapes=[
            pltpu.VMEM((BQ, DM), F32),
            pltpu.VMEM((NWC, BQ, WC), F32),
            pltpu.VMEM((SQ, DM), BF16),
            pltpu.VMEM((N_SUB, BQ, DM), BF16),
            pltpu.VMEM((DM, DM), F32),
            pltpu.VMEM((H, DM, DH), BF16),
            pltpu.VMEM((DM, DM), F32),
            pltpu.VMEM((DM, DM), BF16),
            pltpu.VMEM((H, SKV, DH), F32),
            pltpu.VMEM((H, SKV, DH), F32),
            pltpu.VMEM((H, SKV, DH), BF16),
            pltpu.VMEM((H, SKV, DH), BF16),
            pltpu.VMEM((R1, DM), F32),
            pltpu.VMEM((NL + 1, R1, DH), BF16),
            pltpu.VMEM((R1, DH), F32),
            pltpu.VMEM((R1, DH), F32),
            pltpu.VMEM((N_SUB, BQ, DM), BF16),
            pltpu.VMEM((N_SUB + 1, BQ, DM), BF16),
            pltpu.SemaphoreType.DMA((NP + 2 * NWC + 2 * H + 1,)),
            pltpu.SemaphoreType.DMA((n_ag,)),
            pltpu.SemaphoreType.DMA((n_ag,)),
            pltpu.SemaphoreType.DMA((2 * N_SUB,)),
            pltpu.SemaphoreType.DMA((2 * N_SUB,)),
        ],
        compiler_params=pltpu.CompilerParams(
            collective_id=0,
            vmem_limit_bytes=100 * 1024 * 1024,
            disable_bounds_checks=True,
            disable_semaphore_checks=True,
        ),
    )(x, Wq, K_ext, V_ext, Wo)
```

```python
import jax
import jax.numpy as jnp
from jax import lax
from jax.experimental import pallas as pl
from jax.experimental.pallas import tpu as pltpu

N_DEV = 4
H = 8
DH = 128
SKV = 2048
SQ = 512
DM = 1024
BQ = 256
HB = 128
N_SUB = 6
NP = 4
QB = BQ // NP
NWC = 8
WC = DM // NWC
NL = 5
R1 = SQ + BQ
CUT = 304

QSCALE = 0.08838834764831843 * 1.4426950408889634

_NT = (((1,), (1,)), ((), ()))
BF16 = jnp.bfloat16
F32 = jnp.float32


def _dot(a, b):
    return jnp.dot(a, b, preferred_element_type=F32)


def _cat(parts, axis):
    return parts[0] if len(parts) == 1 else jnp.concatenate(parts, axis=axis)


def _scores(q, k):
    return lax.dot_general(q, k, _NT, preferred_element_type=F32)


def _pv_raw(s, v):
    p = jnp.exp2(s - jnp.max(s, axis=-1, keepdims=True))
    lp = p[:, 0:DH]
    for j in range(1, SKV // DH):
        lp = lp + p[:, j * DH:(j + 1) * DH]
    return _dot(p.astype(BF16), v), lp


def _norm(o, lp):
    l = jnp.sum(lp, axis=-1, keepdims=True)
    r = pl.reciprocal(l, approx=True)
    return (o * (r * (2.0 - l * r))).astype(BF16)


def _kernel(x_hbm, wq_hbm, k_hbm, v_hbm, wo_hbm, out_ref,
            x0f, x1f, xown, xg, wqf, wqb, wof, kf, vf,
            qacc, o1, ou, lp, so, sl, pbuf, rbuf,
            ld_sem, ag_send, ag_recv, rs_send, rs_recv):
    my = lax.axis_index("i")
    left = lax.rem(my + N_DEV - 1, N_DEV)
    right = lax.rem(my + 1, N_DEV)
    h0 = my * H
    hl = H - 1

    def piece_row(i):
        return (i % 2) * HB + (i // 2) * QB

    def x0_copy(i):
        rows = pl.ds(piece_row(i), QB)
        return pltpu.make_async_copy(
            x_hbm.at[0, rows, :], x0f.at[rows, :], ld_sem.at[i])

    def x1_copy(c):
        return pltpu.make_async_copy(
            x_hbm.at[0, pl.ds(BQ, BQ), pl.ds(c * WC, WC)], x1f.at[c],
            ld_sem.at[NP + 2 * c])

    def wq_copy(c):
        rows = pl.ds(c * WC, WC)
        return pltpu.make_async_copy(
            wq_hbm.at[rows, :], wqf.at[rows, :], ld_sem.at[NP + 2 * c + 1])

    def k_copy(h):
        return pltpu.make_async_copy(
            k_hbm.at[0, :, h0 + h, :], kf.at[h], ld_sem.at[NP + 2 * NWC + 2 * h])

    def v_copy(h):
        return pltpu.make_async_copy(
            v_hbm.at[0, :, h0 + h, :], vf.at[h],
            ld_sem.at[NP + 2 * NWC + 2 * h + 1])

    def wo_copy():
        return pltpu.make_async_copy(
            wo_hbm, wof, ld_sem.at[NP + 2 * NWC + 2 * H])

    def remote(src, dst, send_sem, recv_sem, dev):
        return pltpu.make_async_remote_copy(
            src_ref=src, dst_ref=dst, send_sem=send_sem, recv_sem=recv_sem,
            device_id=(dev,), device_id_type=pl.DeviceIdType.MESH)

    def first_copy(i, dev):
        rows = pl.ds(piece_row(i), QB)
        idx = i if i < 2 else 2 * N_SUB + i - 2
        return remote(xown.at[rows, :], xg.at[0, rows, :],
                      ag_send.at[idx], ag_recv.at[idx], dev)

    def ag_copy(src, s, part, dev):
        idx = 2 * s + part
        return remote(src, xg.at[s, pl.ds(part * HB, HB), :],
                      ag_send.at[idx], ag_recv.at[idx], dev)

    def ag_own(stage, u):
        d0, d1 = (left, right) if stage == 0 else (right, left)
        s = 2 * stage + u
        return (ag_copy(xown.at[pl.ds(u * BQ, HB), :], s, 0, d0),
                ag_copy(xown.at[pl.ds(u * BQ + HB, HB), :], s, 1, d1))

    def ag_fwd(u):
        return (ag_copy(xg.at[u, pl.ds(0, HB), :], 2 + u, 0, left),
                ag_copy(xg.at[u, pl.ds(HB, HB), :], 2 + u, 1, right))

    def rs_copy(s, part, dev):
        idx = 2 * s + part
        rows = pl.ds(part * HB, HB)
        return remote(pbuf.at[s, rows, :], rbuf.at[s, rows, :],
                      rs_send.at[idx], rs_recv.at[idx], dev)

    def ag_wait_recv(s):
        for part in range(2):
            ag_copy(xg.at[s, pl.ds(part * HB, HB), :], s, part, my).wait_recv()

    def rs_wait_recv(s):
        for part in range(2):
            rs_copy(s, part, my).wait_recv()

    def kb(h):
        return kf[h].astype(BF16)

    def vb(h):
        return vf[h].astype(BF16)

    def wob(a, b):
        return wof[a * DH:b * DH, :].astype(BF16)

    def q_rows(a, b, h):
        col = h * DH if isinstance(h, int) else pl.multiple_of(h * DH, DH)
        return qacc[a:b, pl.ds(col, DH)].astype(BF16)

    def own_raw(a, b, h):
        return _pv_raw(_scores(q_rows(a, b, h), kb(h)), vb(h))

    def project(a, b):
        return _dot(_cat([_norm(so[h], sl[h]) for h in range(a, b)], -1), wob(a, b))

    def streaming_phase():
        barrier = pltpu.get_barrier_semaphore()
        for nbr in (left, right):
            pl.semaphore_signal(barrier, inc=1, device_id=(nbr,),
                                device_id_type=pl.DeviceIdType.MESH)
        for i in range(NP):
            x0_copy(i).start(priority=1)
        for c in range(NWC):
            x1_copy(c).start(priority=1)
            wq_copy(c).start(priority=1)

        rbuf[N_SUB] = jnp.zeros((BQ, DM), BF16)
        qacc[0:SQ, :] = jnp.zeros((SQ, DM), F32)
        ou[...] = jnp.zeros(ou.shape, F32)
        lp[...] = jnp.ones(lp.shape, F32)

        for i in range(NP):
            x0_copy(i).wait()
            r = piece_row(i)
            xown[r:r + QB, :] = x0f[r:r + QB, :].astype(BF16)
            if i == 0:
                pl.semaphore_wait(barrier, 2)
            first_copy(i, left if i % 2 == 0 else right).start()

        for h in range(H):
            k_copy(h).start(priority=1)
            v_copy(h).start(priority=1)
        wo_copy().start(priority=1)

        def q_chunk(c, carry):
            x1_copy(c).wait()
            wq_copy(c).wait()
            cs = pl.ds(pl.multiple_of(c * WC, WC), WC)
            x1 = x1f[c].astype(BF16)
            xown[BQ:SQ, cs] = x1
            w = (wqf[cs, :] * QSCALE).astype(BF16)
            for h in range(H):
                wqb[h, cs, :] = w[:, h * DH:(h + 1) * DH]
            xc = jnp.concatenate([xown[0:BQ, cs], x1], axis=0)
            qacc[0:SQ, :] = qacc[0:SQ, :] + _dot(xc, w)
            return carry

        lax.fori_loop(0, NWC, q_chunk, 0)

        for i in range(NP):
            first_copy(i, my).wait_recv()
        for c in ag_own(0, 1) + ag_fwd(0):
            c.start()
        qacc[SQ:R1, 0:hl * DH] = _dot(xg[0], _cat([wqb[h] for h in range(hl)], -1))

        def wait_kv(h):
            k_copy(h).wait()
            v_copy(h).wait()

        def head(h, carry):
            wait_kv(h)
            o1[h] = _norm(ou[...], lp[...])
            ou[0:CUT, :], lp[0:CUT, :] = own_raw(0, CUT, h)
            o, l = own_raw(CUT, R1, h)
            ou[CUT:SQ, :] = o[0:SQ - CUT]
            lp[CUT:SQ, :] = l[0:SQ - CUT]
            so[h] = o[SQ - CUT:]
            sl[h] = l[SQ - CUT:]
            return carry

        lax.fori_loop(0, NL, head, 0)

        for c in ag_own(2, 0) + ag_own(2, 1):
            c.start()
        for h in range(NL, H):
            wait_kv(h)
        q_last = _dot(xg[0], wqb[hl]).astype(BF16)
        for h in range(NL, hl):
            so[h], sl[h] = own_raw(SQ, R1, h)
        so[hl], sl[hl] = _pv_raw(_scores(q_last, kb(hl)), vb(hl))
        wo_copy().wait()

    def sub_block(s, carry):
        ag_wait_recv(s)

        @pl.when(s == 1)
        def _():
            for c in ag_fwd(1):
                c.start()

        @pl.when(s == 5)
        def _():
            rs_wait_recv(2)

        x = xg[s]
        q = [_dot(x, wqb[h]).astype(BF16) for h in range(2)]
        y = rbuf[jnp.where(s == 5, 2, N_SUB)].astype(F32) + project(0, hl)
        for h in range(H):
            sc = _scores(q[h], kb(h))
            if 1 <= h < hl:
                q.append(_dot(x, wqb[h + 1]).astype(BF16))
            if h == hl:
                y = y + project(hl, H)
            so[h], sl[h] = _pv_raw(sc, vb(h))
        pbuf[s - 1] = y.astype(BF16)
        first = s < 3
        rs_copy(s - 1, 0, jnp.where(first, right, left)).start()
        rs_copy(s - 1, 1, jnp.where(first, left, right)).start()
        return carry

    def steady_phase():
        lax.fori_loop(1, N_SUB, sub_block, 0)
        for s in (0, 1, 3):
            rs_wait_recv(s)
        y = _dot(o1[1], wob(0, 1))
        out_ref[0, 0:BQ, :] = y[0:BQ] + rbuf[0].astype(F32)
        out_ref[0, BQ:SQ, :] = y[BQ:SQ] + rbuf[1].astype(F32)
        pbuf[5] = (rbuf[3].astype(F32) + project(0, H)).astype(BF16)
        o1[NL] = _norm(ou[...], lp[...])
        rs_copy(5, 0, left).start()
        rs_copy(5, 1, right).start()

    def own_phase():
        y = out_ref[0] + _dot(o1[2], wob(1, 2))
        o = [o1[h + 1] for h in range(3, NL)]
        o.append(_cat([_norm(*own_raw(0, BQ, NL)), _norm(*own_raw(BQ, SQ, NL))], 0))
        o += [_norm(*own_raw(0, SQ, h)) for h in range(NL + 1, hl)]
        ou[...], lp[...] = own_raw(0, SQ, hl)
        out_ref[0] = y + _dot(_cat(o, -1), wob(3, hl))

        for i in range(NP):
            first_copy(i, my).wait_send()
        for c in (ag_own(0, 1) + ag_own(2, 0) + ag_own(2, 1)
                  + ag_fwd(0) + ag_fwd(1)):
            c.wait_send()
        for s in range(N_SUB):
            for part in range(2):
                rs_copy(s, part, my).wait_send()
        rs_wait_recv(4)
        rs_wait_recv(5)
        y = out_ref[0] + _dot(o1[3], wob(2, 3))
        y = y + _dot(_norm(ou[...], lp[...]), wob(hl, H))
        out_ref[0, 0:BQ, :] = y[0:BQ] + rbuf[4].astype(F32)
        out_ref[0, BQ:SQ, :] = y[BQ:SQ] + rbuf[5].astype(F32)

    def phase(i, carry):
        pl.when(i == 0)(streaming_phase)
        pl.when(i == 1)(steady_phase)
        pl.when(i == 2)(own_phase)
        return carry

    lax.fori_loop(0, 3, phase, 0)


def pallas_dist_attn_cross_mha_kvrep_htp_ss_b1_sq512_skv2048_d1024_hq8_dh128_kernel(
    x: jax.Array,
    Wq: jax.Array,
    K_ext: jax.Array,
    V_ext: jax.Array,
    Wo: jax.Array,
):
    any_spec = pl.BlockSpec(memory_space=pl.ANY)
    n_ag = 2 * N_SUB + NP - 2
    return pl.pallas_call(
        _kernel,
        out_shape=jax.ShapeDtypeStruct((1, SQ, DM), F32),
        in_specs=[any_spec] * 5,
        out_specs=pl.BlockSpec(memory_space=pltpu.VMEM),
        scratch_shapes=[
            pltpu.VMEM((BQ, DM), F32),
            pltpu.VMEM((NWC, BQ, WC), F32),
            pltpu.VMEM((SQ, DM), BF16),
            pltpu.VMEM((N_SUB, BQ, DM), BF16),
            pltpu.VMEM((DM, DM), F32),
            pltpu.VMEM((H, DM, DH), BF16),
            pltpu.VMEM((DM, DM), F32),
            pltpu.VMEM((H, SKV, DH), F32),
            pltpu.VMEM((H, SKV, DH), F32),
            pltpu.VMEM((R1, DM), F32),
            pltpu.VMEM((NL + 1, SQ, DH), BF16),
            pltpu.VMEM((SQ, DH), F32),
            pltpu.VMEM((SQ, DH), F32),
            pltpu.VMEM((H, BQ, DH), F32),
            pltpu.VMEM((H, BQ, DH), F32),
            pltpu.VMEM((N_SUB, BQ, DM), BF16),
            pltpu.VMEM((N_SUB + 1, BQ, DM), BF16),
            pltpu.SemaphoreType.DMA((NP + 2 * NWC + 2 * H + 1,)),
            pltpu.SemaphoreType.DMA((n_ag,)),
            pltpu.SemaphoreType.DMA((n_ag,)),
            pltpu.SemaphoreType.DMA((2 * N_SUB,)),
            pltpu.SemaphoreType.DMA((2 * N_SUB,)),
        ],
        compiler_params=pltpu.CompilerParams(
            collective_id=0,
            vmem_limit_bytes=100 * 1024 * 1024,
            disable_semaphore_checks=True,
        ),
    )(x, Wq, K_ext, V_ext, Wo)
```

```python
import jax
import jax.numpy as jnp
from jax import lax
from jax.experimental import pallas as pl
from jax.experimental.pallas import tpu as pltpu

N_DEV = 4
H = 8
DH = 128
SKV = 2048
SQ = 512
DM = 1024
BQ = 256
HB = 128
N_SUB = 6
NP = 4
QB = BQ // NP
NWC = 8
WC = DM // NWC
NL = 5
R1 = SQ + BQ
CUT = 304

QSCALE = 0.08838834764831843 * 1.4426950408889634

_NT = (((1,), (1,)), ((), ()))
BF16 = jnp.bfloat16
F32 = jnp.float32


def _dot(a, b):
    return jnp.dot(a, b, preferred_element_type=F32)


def _cat(parts, axis):
    return parts[0] if len(parts) == 1 else jnp.concatenate(parts, axis=axis)


def _scores(q, k):
    return lax.dot_general(q, k, _NT, preferred_element_type=F32)


def _pv_raw(s, v):
    p = jnp.exp2(s - jnp.max(s, axis=-1, keepdims=True))
    lp = p[:, 0:DH]
    for j in range(1, SKV // DH):
        lp = lp + p[:, j * DH:(j + 1) * DH]
    return _dot(p.astype(BF16), v), lp


def _norm(o, lp):
    l = jnp.sum(lp, axis=-1, keepdims=True)
    r = pl.reciprocal(l, approx=True)
    return (o * (r * (2.0 - l * r))).astype(BF16)


def _kernel(x_hbm, wq_hbm, k_hbm, v_hbm, wo_hbm, out_ref,
            x0f, x1f, xown, xg, wqf, wqb, wof, kf, vf,
            qacc, o1, ou, lp, so, sl, pbuf, rbuf,
            ld_sem, ag_send, ag_recv, rs_send, rs_recv):
    my = lax.axis_index("i")
    left = lax.rem(my + N_DEV - 1, N_DEV)
    right = lax.rem(my + 1, N_DEV)
    h0 = my * H
    hl = H - 1

    def piece_row(i):
        return (i % 2) * HB + (i // 2) * QB

    def x0_copy(i):
        rows = pl.ds(piece_row(i), QB)
        return pltpu.make_async_copy(
            x_hbm.at[0, rows, :], x0f.at[rows, :], ld_sem.at[i])

    def x1_copy(c):
        return pltpu.make_async_copy(
            x_hbm.at[0, pl.ds(BQ, BQ), pl.ds(c * WC, WC)], x1f.at[c],
            ld_sem.at[NP + 2 * c])

    def wq_copy(c):
        rows = pl.ds(c * WC, WC)
        return pltpu.make_async_copy(
            wq_hbm.at[rows, :], wqf.at[rows, :], ld_sem.at[NP + 2 * c + 1])

    def k_copy(h):
        return pltpu.make_async_copy(
            k_hbm.at[0, :, h0 + h, :], kf.at[h], ld_sem.at[NP + 2 * NWC + 2 * h])

    def v_copy(h):
        return pltpu.make_async_copy(
            v_hbm.at[0, :, h0 + h, :], vf.at[h],
            ld_sem.at[NP + 2 * NWC + 2 * h + 1])

    def wo_copy():
        return pltpu.make_async_copy(
            wo_hbm, wof, ld_sem.at[NP + 2 * NWC + 2 * H])

    def remote(src, dst, send_sem, recv_sem, dev):
        return pltpu.make_async_remote_copy(
            src_ref=src, dst_ref=dst, send_sem=send_sem, recv_sem=recv_sem,
            device_id=(dev,), device_id_type=pl.DeviceIdType.MESH)

    def first_copy(i, dev):
        rows = pl.ds(piece_row(i), QB)
        idx = i if i < 2 else 2 * N_SUB + i - 2
        return remote(xown.at[rows, :], xg.at[0, rows, :],
                      ag_send.at[idx], ag_recv.at[idx], dev)

    def ag_copy(src, s, part, dev):
        idx = 2 * s + part
        return remote(src, xg.at[s, pl.ds(part * HB, HB), :],
                      ag_send.at[idx], ag_recv.at[idx], dev)

    def ag_own(stage, u):
        d0, d1 = (left, right) if stage == 0 else (right, left)
        s = 2 * stage + u
        return (ag_copy(xown.at[pl.ds(u * BQ, HB), :], s, 0, d0),
                ag_copy(xown.at[pl.ds(u * BQ + HB, HB), :], s, 1, d1))

    def ag_fwd(u):
        return (ag_copy(xg.at[u, pl.ds(0, HB), :], 2 + u, 0, left),
                ag_copy(xg.at[u, pl.ds(HB, HB), :], 2 + u, 1, right))

    def rs_copy(s, part, dev):
        idx = 2 * s + part
        rows = pl.ds(part * HB, HB)
        return remote(pbuf.at[s, rows, :], rbuf.at[s, rows, :],
                      rs_send.at[idx], rs_recv.at[idx], dev)

    def ag_wait_recv(s):
        for part in range(2):
            ag_copy(xg.at[s, pl.ds(part * HB, HB), :], s, part, my).wait_recv()

    def rs_wait_recv(s):
        for part in range(2):
            rs_copy(s, part, my).wait_recv()

    def kb(h):
        return kf[h].astype(BF16)

    def vb(h):
        return vf[h].astype(BF16)

    def wob(a, b):
        return wof[a * DH:b * DH, :].astype(BF16)

    def q_rows(a, b, h):
        col = h * DH if isinstance(h, int) else pl.multiple_of(h * DH, DH)
        return (qacc[a:b, pl.ds(col, DH)] * QSCALE).astype(BF16)

    def q_head(x, h):
        return (_dot(x, wqb[h]) * QSCALE).astype(BF16)

    def own_raw(a, b, h):
        return _pv_raw(_scores(q_rows(a, b, h), kb(h)), vb(h))

    def project(a, b):
        return _dot(_cat([_norm(so[h], sl[h]) for h in range(a, b)], -1), wob(a, b))

    def streaming_phase():
        barrier = pltpu.get_barrier_semaphore()
        for nbr in (left, right):
            pl.semaphore_signal(barrier, inc=1, device_id=(nbr,),
                                device_id_type=pl.DeviceIdType.MESH)
        for i in range(NP):
            x0_copy(i).start(priority=1)
        for c in range(NWC):
            x1_copy(c).start(priority=1)
            wq_copy(c).start(priority=1)

        rbuf[N_SUB] = jnp.zeros((BQ, DM), BF16)
        qacc[0:SQ, :] = jnp.zeros((SQ, DM), F32)
        ou[...] = jnp.zeros(ou.shape, F32)
        lp[...] = jnp.ones(lp.shape, F32)

        for i in range(NP):
            x0_copy(i).wait()
            r = piece_row(i)
            xown[r:r + QB, :] = x0f[r:r + QB, :].astype(BF16)
            if i == 0:
                pl.semaphore_wait(barrier, 2)
            first_copy(i, left if i % 2 == 0 else right).start()

        for h in range(H):
            k_copy(h).start(priority=1)
            v_copy(h).start(priority=1)
        wo_copy().start(priority=1)

        def q_chunk(c, carry):
            x1_copy(c).wait()
            wq_copy(c).wait()
            cs = pl.ds(pl.multiple_of(c * WC, WC), WC)
            x1 = x1f[c].astype(BF16)
            xown[BQ:SQ, cs] = x1
            xc = jnp.concatenate([xown[0:BQ, cs], x1], axis=0)
            qacc[0:SQ, :] = qacc[0:SQ, :] + _dot(xc, wqf[cs, :].astype(BF16))
            for h in range(H):
                wqb[h, cs, :] = wqf[cs, h * DH:(h + 1) * DH].astype(BF16)
            return carry

        lax.fori_loop(0, NWC, q_chunk, 0)

        for i in range(NP):
            first_copy(i, my).wait_recv()
        for c in ag_own(0, 1) + ag_fwd(0):
            c.start()
        qacc[SQ:R1, 0:hl * DH] = _dot(xg[0], _cat([wqb[h] for h in range(hl)], -1))

        def wait_kv(h):
            k_copy(h).wait()
            v_copy(h).wait()

        def head(h, carry):
            wait_kv(h)
            o1[h] = _norm(ou[...], lp[...])
            ou[0:CUT, :], lp[0:CUT, :] = own_raw(0, CUT, h)
            o, l = own_raw(CUT, R1, h)
            ou[CUT:SQ, :] = o[0:SQ - CUT]
            lp[CUT:SQ, :] = l[0:SQ - CUT]
            so[h] = o[SQ - CUT:]
            sl[h] = l[SQ - CUT:]
            return carry

        lax.fori_loop(0, NL, head, 0)

        for c in ag_own(2, 0) + ag_own(2, 1):
            c.start()
        for h in range(NL, H):
            wait_kv(h)
        q_last = q_head(xg[0], hl)
        for h in range(NL, hl):
            so[h], sl[h] = own_raw(SQ, R1, h)
        so[hl], sl[hl] = _pv_raw(_scores(q_last, kb(hl)), vb(hl))
        wo_copy().wait()

    def sub_block(s, carry):
        ag_wait_recv(s)

        @pl.when(s == 1)
        def _():
            for c in ag_fwd(1):
                c.start()

        @pl.when(s == 5)
        def _():
            rs_wait_recv(2)

        x = xg[s]
        q = [q_head(x, h) for h in range(2)]
        y = rbuf[jnp.where(s == 5, 2, N_SUB)].astype(F32) + project(0, hl)
        for h in range(H):
            sc = _scores(q[h], kb(h))
            if 1 <= h < hl:
                q.append(q_head(x, h + 1))
            if h == hl:
                y = y + project(hl, H)
            so[h], sl[h] = _pv_raw(sc, vb(h))
        pbuf[s - 1] = y.astype(BF16)
        first = s < 3
        rs_copy(s - 1, 0, jnp.where(first, right, left)).start()
        rs_copy(s - 1, 1, jnp.where(first, left, right)).start()
        return carry

    def steady_phase():
        lax.fori_loop(1, N_SUB, sub_block, 0)
        for s in (0, 1, 3):
            rs_wait_recv(s)
        y = _dot(o1[1], wob(0, 1))
        out_ref[0, 0:BQ, :] = y[0:BQ] + rbuf[0].astype(F32)
        out_ref[0, BQ:SQ, :] = y[BQ:SQ] + rbuf[1].astype(F32)
        pbuf[5] = (rbuf[3].astype(F32) + project(0, H)).astype(BF16)
        o1[NL] = _norm(ou[...], lp[...])
        rs_copy(5, 0, left).start()
        rs_copy(5, 1, right).start()

    def own_phase():
        y = out_ref[0] + _dot(o1[2], wob(1, 2))
        for g in range(2):
            so[g], sl[g] = own_raw(g * BQ, (g + 1) * BQ, NL)
        for h in range(NL + 1, H):
            o, l = own_raw(0, SQ, h)
            for g in range(2):
                so[2 * (h - NL) + g] = o[g * BQ:(g + 1) * BQ]
                sl[2 * (h - NL) + g] = l[g * BQ:(g + 1) * BQ]
        out_ref[0] = y + _dot(
            _cat([o1[h + 1] for h in range(3, NL)], -1), wob(3, NL))

        for i in range(NP):
            first_copy(i, my).wait_send()
        for c in (ag_own(0, 1) + ag_own(2, 0) + ag_own(2, 1)
                  + ag_fwd(0) + ag_fwd(1)):
            c.wait_send()
        for s in range(N_SUB):
            for part in range(2):
                rs_copy(s, part, my).wait_send()
        rs_wait_recv(4)
        rs_wait_recv(5)
        y = out_ref[0] + _dot(o1[3], wob(2, 3))
        o = [_cat([_norm(so[2 * j + g], sl[2 * j + g]) for g in range(2)], 0)
             for j in range(H - NL)]
        y = y + _dot(_cat(o, -1), wob(NL, H))
        out_ref[0, 0:BQ, :] = y[0:BQ] + rbuf[4].astype(F32)
        out_ref[0, BQ:SQ, :] = y[BQ:SQ] + rbuf[5].astype(F32)

    def phase(i, carry):
        pl.when(i == 0)(streaming_phase)
        pl.when(i == 1)(steady_phase)
        pl.when(i == 2)(own_phase)
        return carry

    lax.fori_loop(0, 3, phase, 0)


def pallas_dist_attn_cross_mha_kvrep_htp_ss_b1_sq512_skv2048_d1024_hq8_dh128_kernel(
    x: jax.Array,
    Wq: jax.Array,
    K_ext: jax.Array,
    V_ext: jax.Array,
    Wo: jax.Array,
):
    any_spec = pl.BlockSpec(memory_space=pl.ANY)
    n_ag = 2 * N_SUB + NP - 2
    return pl.pallas_call(
        _kernel,
        out_shape=jax.ShapeDtypeStruct((1, SQ, DM), F32),
        in_specs=[any_spec] * 5,
        out_specs=pl.BlockSpec(memory_space=pltpu.VMEM),
        scratch_shapes=[
            pltpu.VMEM((BQ, DM), F32),
            pltpu.VMEM((NWC, BQ, WC), F32),
            pltpu.VMEM((SQ, DM), BF16),
            pltpu.VMEM((N_SUB, BQ, DM), BF16),
            pltpu.VMEM((DM, DM), F32),
            pltpu.VMEM((H, DM, DH), BF16),
            pltpu.VMEM((DM, DM), F32),
            pltpu.VMEM((H, SKV, DH), F32),
            pltpu.VMEM((H, SKV, DH), F32),
            pltpu.VMEM((R1, DM), F32),
            pltpu.VMEM((NL + 1, SQ, DH), BF16),
            pltpu.VMEM((SQ, DH), F32),
            pltpu.VMEM((SQ, DH), F32),
            pltpu.VMEM((H, BQ, DH), F32),
            pltpu.VMEM((H, BQ, DH), F32),
            pltpu.VMEM((N_SUB, BQ, DM), BF16),
            pltpu.VMEM((N_SUB + 1, BQ, DM), BF16),
            pltpu.SemaphoreType.DMA((NP + 2 * NWC + 2 * H + 1,)),
            pltpu.SemaphoreType.DMA((n_ag,)),
            pltpu.SemaphoreType.DMA((n_ag,)),
            pltpu.SemaphoreType.DMA((2 * N_SUB,)),
            pltpu.SemaphoreType.DMA((2 * N_SUB,)),
        ],
        compiler_params=pltpu.CompilerParams(
            collective_id=0,
            vmem_limit_bytes=100 * 1024 * 1024,
            disable_semaphore_checks=True,
        ),
    )(x, Wq, K_ext, V_ext, Wo)
```
